```python
import numpy as np

kernel_name = "dist_sparse_attn_blocksparse_qseq_b2_sq256_skv256_hq4_dh64"

def setup_inputs():
    x = np.random.randn(2, 1024, 512).astype(np.float32)
    Wq = np.random.randn(512, 1024).astype(np.float32) * 0.02
    K_ext = np.random.randn(2, 256, 16, 64).astype(np.float32)
    V_ext = np.random.randn(2, 256, 16, 64).astype(np.float32)
    Wo = np.random.randn(1024, 512).astype(np.float32) * 0.02
    return {"x": x, "Wq": Wq, "K_ext": K_ext, "V_ext": V_ext, "Wo": Wo}

def reference(x, Wq, K_ext, V_ext, Wo):
    B, Sq, Skv, Hq, Dh = 2, 1024, 256, 16, 64
    Q = (x @ Wq).reshape(B, Sq, Hq, Dh)
    qb = (np.arange(Sq) // 64)[:, None]
    kb = (np.arange(Skv) // 64)[None, :]
    mask = (qb == kb) | (kb == 0) | ((qb + kb) % 3 == 0)
    scores = np.einsum('bihd,bjhd->bhij', Q, K_ext).astype(np.float32) * 0.125
    scores = np.where(mask[None, None, :, :], scores, -1e9)
    scores_max = scores.max(axis=-1, keepdims=True)
    w = np.exp(scores - scores_max)
    row_keep = mask.any(axis=1)
    w_sum = np.where(row_keep[None, None, :, None], w.sum(axis=-1, keepdims=True), 1.0)
    w = w / w_sum
    w = np.where(row_keep[None, None, :, None], w, 0.0)
    ctx = np.einsum('bhij,bjhd->bihd', w, V_ext).reshape(B, Sq, Hq * Dh)
    return ctx @ Wo
```

```python
import numpy as np
import jax
import jax.numpy as jnp
from jax import lax
from jax.experimental import pallas as pl
from jax.experimental.pallas import tpu as pltpu

N_DEV = 4
B, SQ, SKV, DH, DM = 2, 256, 256, 64, 512
ROWS = B * SQ
HALF = 2 * DH
BLK = 64
MESH = pl.DeviceIdType.MESH
bf16 = jnp.bfloat16
f32 = jnp.float32
i32 = jnp.int32
NT = (((1,), (1,)), ((), ()))

R0 = 32
RE = 128
UQ = ((0, RE), (RE, 256), (256, 512))
U0, U1, U2, V0, V1 = range(5)
NQ = (RE // 64, (256 - RE) // 64, 4, 4, 4)
HD = 5


def _c(v):
    return jnp.int32(np.uint32(v).astype(np.int32))


def _srl(x, n):
    return lax.shift_right_logical(x, jnp.full(x.shape, n, i32))


def _sll(x, n):
    return lax.shift_left(x, jnp.full(x.shape, n, i32))


def _encode(x):
    n = x.shape[0] // 2
    w = pltpu.bitcast(x, i32)
    mag = w & _c(0x7FFF7FFF)
    hi = _srl(mag, 16)
    lo = mag & _c(0x7FFF)
    mx = jnp.max(jnp.maximum(hi, lo), axis=0, keepdims=True)
    base = jnp.maximum(mx - 2047, 0)
    th = jnp.maximum(hi - base, 0)
    tl = jnp.maximum(lo - base, 0)
    code = tl | _sll(th, 16) | (_srl(w, 4) & _c(0x08000800))
    isx = jnp.minimum((hi - 1) & 0x7FFF, (lo - 1) & 0x7FFF) < base
    rid = lax.broadcasted_iota(i32, (n, 128), 0) + 1
    v = jnp.where(isx, rid, 0)
    imax = jnp.max(v, axis=0, keepdims=True)
    isum = jnp.sum(v, axis=0, keepdims=True)
    imin = jnp.min(jnp.where(isx, rid, 255), axis=0, keepdims=True)
    bad = jnp.where(isum > imax + imin, 1, 0)
    w1 = jnp.sum(jnp.where(rid == imax, w, 0), axis=0, keepdims=True)
    w2 = jnp.sum(jnp.where(rid == imin, w, 0), axis=0, keepdims=True)
    hdr = base | _sll(imax, 15) | _sll(imin, 23) | _sll(bad, 31)
    out = []
    for q in range(n // 32):
        e = code[32 * q + 24:32 * q + 32]
        for j in range(3):
            out.append(code[32 * q + 8 * j:32 * q + 8 * j + 8] | (_sll(e, 12 - 4 * j) & _c(0xF000F000)))
    return jnp.concatenate([w1, w2, hdr], axis=0), jnp.concatenate(out, axis=0)


def _decode(head, body, q0=0):
    k = body.shape[0] // 24
    w1, w2, hdr = head[0:1], head[1:2], head[2:3]
    base = hdr & 0x7FFF
    base2 = base | _sll(base, 16)
    imax = _srl(hdr, 15) & 0xFF
    imin = _srl(hdr, 23) & 0xFF
    g = []
    for q in range(k):
        c = [body[24 * q + 8 * j:24 * q + 8 * j + 8] for j in range(3)]
        e = None
        for j in range(3):
            f = _srl(c[j], 12 - 4 * j) & _c(0x000F000F << (4 * j))
            e = f if e is None else e | f
        g += c + [e]
    c = jnp.concatenate(g, axis=0)
    t = c & _c(0x07FF07FF)
    m = (t + _c(0x07FF07FF)) & _c(0x08000800)
    mask = _sll(m, 4) - _srl(m, 11)
    w = (t + (base2 & mask)) | (_sll(c, 4) & _c(0x80008000))
    rid = lax.broadcasted_iota(i32, (32 * k, 128), 0) + (32 * q0 + 1)
    w = jnp.where(rid == imax, w1, jnp.where(rid == imin, w2, w))
    return pltpu.bitcast(w, bf16)


def _body(x_hbm, wq_hbm, kt_hbm, vt_hbm, wo_hbm, out_ref,
          x_f, x_b, wq_f, wo_f, wq_o, wo_o, head_q, pk, kt_f, vt_f, ctx, stage, c_tmp, lhs_t,
          raw_q, raw_o,
          lsem, ssem, rsem, ready, fsem_s, fsem_r):
    p = lax.axis_index("i")
    left = (p + 3) % N_DEV
    right = (p + 1) % N_DEV
    diag = (p + 2) % N_DEV
    scope = jax.named_scope
    A, Bh = 0, 1

    nl = [0]

    def local(src, dst):
        cp = pltpu.make_async_copy(src, dst, lsem.at[nl[0]])
        nl[0] += 1
        cp.start()
        return cp

    nr = [0]

    def rc(src, dst, tgt):
        idx = nr[0]
        nr[0] += 1
        return pltpu.make_async_remote_copy(src, dst, ssem.at[idx], rsem.at[idx],
                                            device_id=(tgt,), device_id_type=MESH)

    def plan(tgt, h1, ds):
        def unit(ss, sd, h, u, qa=0, qb=None):
            qb = NQ[u] if qb is None else qb
            lo = HD if qa == 0 else 8 + 24 * qa
            r = pl.ds(lo, 8 + 24 * qb - lo)
            return rc(pk.at[ss, h, u, r], pk.at[sd, h, u, r], tgt)
        h2 = 1 - h1
        d = {}
        d["q0"] = rc(wq_hbm.at[pl.ds(0, R0), pl.ds(h1 * HALF, HALF)], stage.at[ds - 1], tgt)
        d["qr"] = rc(wq_o.at[h1, pl.ds(R0, RE - R0)], head_q.at[ds - 1, pl.ds(R0, RE - R0)], tgt)
        for h in range(2):
            d["u1", h] = unit(0, ds, h, U1)
            d["u2", h] = unit(0, ds, h, U2)
        d["u0"] = unit(0, ds, h2, U0)
        d["o1"] = [unit(0, ds, h1, u) for u in (V0, V1)]
        d["fq"] = [unit(ds, 3, h1, u) for u in (U1, U2, U0)]
        d["o2"] = [unit(0, ds, h2, u) for u in (V0, V1)]
        d["fo"] = [unit(ds, 3, h1, V0), unit(ds, 3, h1, V1, 0, 2), unit(ds, 3, h1, V1, 2, 3),
                   unit(ds, 3, h1, V1, 3, 4)]
        return d
    R = plan(right, A, 1)
    L = plan(left, Bh, 2)
    DIRS = ((R, 1, A), (L, 2, Bh))

    bar = pltpu.get_barrier_semaphore()

    def sig(sem, tgt):
        pl.semaphore_signal(sem, inc=1, device_id=(tgt,), device_id_type=MESH)
    early_R = jnp.logical_or(p == 2, p == 3)
    early_L = jnp.logical_or(p == 1, p == 2)

    @pl.when(p == 0)
    def _():
        sig(bar, right)
        sig(bar, left)

    @pl.when(p == 1)
    def _():
        sig(bar, right)
        pl.semaphore_wait(bar, 1)
        L["q0"].start()
        sig(ready.at[0], left)

    @pl.when(p == 3)
    def _():
        sig(bar, left)
        pl.semaphore_wait(bar, 1)
        R["q0"].start()
        sig(ready.at[1], right)

    groups = (p, left, right, diag)

    def kv(s, h):
        rows = pl.ds(pl.multiple_of(groups[s] * 256 + h * HALF, HALF), HALF)
        dst = pl.ds(h * HALF, HALF)
        return [local(kt_hbm.at[:, rows, :], kt_f.at[s, :, dst, :]),
                local(vt_hbm.at[:, rows, :], vt_f.at[s, :, dst, :])]

    WQC = ((R0, RE), (RE, 256), (256, 512), (0, R0))
    c_wq = [local(wq_hbm.at[pl.ds(a, b - a)], wq_f.at[pl.ds(a, b - a)]) for a, b in WQC]
    own_rows = pl.ds(pl.multiple_of(p * 256, 256), 256)
    c_x0 = local(x_hbm.at[pl.ds(0, SQ)], x_f.at[pl.ds(0, SQ)])
    c_kv0 = [local(kt_hbm.at[0, own_rows, :], kt_f.at[0, 0]),
             local(vt_hbm.at[0, own_rows, :], vt_f.at[0, 0])]
    c_wo = local(wo_hbm, wo_f)
    c_x1 = local(x_hbm.at[pl.ds(SQ, SQ)], x_f.at[pl.ds(SQ, SQ)])
    c_kv1 = [local(kt_hbm.at[1, own_rows, :], kt_f.at[0, 1]),
             local(vt_hbm.at[1, own_rows, :], vt_f.at[0, 1])]
    c_kv = {}
    for sh in ((1, A), (2, Bh), (1, Bh), (2, A), (3, A), (3, Bh)):
        c_kv[sh] = kv(*sh)

    @pl.when(p == 2)
    def _():
        pl.semaphore_wait(bar, 2)
        sig(ready.at[1], right)
        sig(ready.at[0], left)
        R["q0"].start()
        L["q0"].start()

    flags = []

    def enc(x, s, h, u):
        head, body = _encode(x)
        pk[s, h, u, HD:8, :] = head
        pk[s, h, u, 8:8 + 24 * NQ[u], :] = body
        flags.append(head[2:3])

    def dec(s, h, u, qa=0, qb=None):
        qb = NQ[u] if qb is None else qb
        head = pk[s, h, u, HD:8, :]
        if qa == 0:
            flags.append(head[2:3])
        return _decode(head, pk[s, h, u, 8 + 24 * qa:8 + 24 * qb, :], qa)

    def early(fn):
        @pl.when(early_R)
        def _():
            fn(R, A)

        @pl.when(early_L)
        def _():
            fn(L, Bh)

    def cast_wq(k):
        a, b = WQC[k]
        c_wq[k].wait()
        for h in range(2):
            wq_o[h, a:b, :] = wq_f[a:b, h * HALF:(h + 1) * HALF].astype(bf16)

    def start(*cps):
        for c in cps:
            c.start()

    with scope("prep_wq"):
        cast_wq(0)
        early(lambda d, h1: start(d["qr"]))
        cast_wq(1)
        for h in range(2):
            enc(wq_o[h, UQ[U1][0]:UQ[U1][1], :], 0, h, U1)
            early(lambda d, h1: start(d["u1", h]))
        cast_wq(2)
        for h in range(2):
            enc(wq_o[h, UQ[U2][0]:UQ[U2][1], :], 0, h, U2)
        early(lambda d, h1: start(d["u2", h1], d["u2", 1 - h1]))
        cast_wq(3)
        for h in range(2):
            enc(wq_o[h, UQ[U0][0]:UQ[U0][1], :], 0, h, U0)
        early(lambda d, h1: start(d["u0"]))

    with scope("ready"):
        def late(d, h1):
            for key in ("qr", "q0", ("u1", h1), ("u2", h1), ("u1", 1 - h1), ("u2", 1 - h1), "u0"):
                d[key].start()

        @pl.when(jnp.logical_not(early_R))
        def _():
            pl.semaphore_wait(ready.at[0], 1)
            late(R, A)

        @pl.when(jnp.logical_not(early_L))
        def _():
            pl.semaphore_wait(ready.at[1], 1)
            late(L, Bh)

    Xs = [3 - lax.rem(p + j, 3) for j in range(3)]
    en = p == 0
    NINF = -jnp.inf
    QSCALE = 0.125 * 1.4426950408889634
    rows = [(0, 128), (128, 192), (192, 256)]

    def bd(w):
        z = jnp.zeros((32, HALF), i32)
        top = jnp.concatenate([w[0:32], z], axis=1)
        bot = jnp.concatenate([z, w[32:64]], axis=1)
        return pltpu.bitcast(jnp.concatenate([top, bot], axis=0), bf16)

    def tiles(t):
        w = pltpu.bitcast(t.astype(bf16), i32)
        t0, t1 = w[:, 0:HALF], w[:, HALF:2 * HALF]
        return t0, t1, pltpu.roll(t1, DH, 1)

    def sel(t, X):
        lane = lax.broadcasted_iota(i32, (64, HALF), 1)
        keep = lane < jnp.where(X == 1, HALF, DH)
        return jnp.where(keep, t[0], jnp.where(X == 3, t[1], t[2]))

    def ex(t):
        lo32 = lax.broadcasted_iota(i32, (32, HALF), 1) < DH
        rt0 = pltpu.roll(t[0][0:32], DH, 1)
        e1 = jnp.concatenate([jnp.where(lo32, rt0, 0), jnp.where(lo32, 0, t[0][32:64])], axis=0)
        e2 = jnp.concatenate([jnp.where(lo32, t[1][0:32], 0), jnp.where(lo32, 0, t[2][32:64])], axis=0)
        return pltpu.bitcast(e1, bf16), pltpu.bitcast(e2, bf16)

    def scores(b, wq, kt):
        q = jnp.dot(x_b[b * SQ:(b + 1) * SQ, :], wq, preferred_element_type=f32) * QSCALE
        kts = tiles(kt)
        qg = [jnp.concatenate([q[0:BLK], q[3 * BLK:4 * BLK]], axis=0).astype(bf16),
              q[BLK:2 * BLK].astype(bf16), q[2 * BLK:3 * BLK].astype(bf16)]
        s = jnp.concatenate([jnp.dot(qg[g], bd(sel(kts, Xs[g])), preferred_element_type=f32)
                             for g in range(3)], axis=0)
        ek = ex(kts)
        sc = jnp.concatenate([jnp.dot(qg[1], ek[0], preferred_element_type=f32),
                              jnp.dot(qg[2], ek[1], preferred_element_type=f32)], axis=0)
        return s, jnp.where(en, sc, NINF)

    def finish(ss, vt):
        s, sc = ss
        vts = tiles(vt)
        ev = ex(vts)
        s1, s2 = s[:, :HALF], s[:, HALF:]
        lo = lax.broadcasted_iota(i32, (SQ, HALF), 1) < DH
        lom = lo[0:128]
        x1 = jnp.concatenate([s1[0:128], jnp.maximum(s1[128:256], jnp.where(lom, sc, NINF))], axis=0)
        x2 = jnp.concatenate([s2[0:128], jnp.maximum(s2[128:256], jnp.where(lom, NINF, sc))], axis=0)
        m1 = jnp.max(x1, axis=-1, keepdims=True)
        m2 = jnp.max(x2, axis=-1, keepdims=True)
        e1 = jnp.exp2(s1 - m1)
        e2 = jnp.exp2(s2 - m2)
        ec = jnp.exp2(sc - jnp.where(lom, m1[128:256], m2[128:256]))
        y1 = jnp.concatenate([e1[0:128], e1[128:256] + jnp.where(lom, ec, 0.0)], axis=0)
        y2 = jnp.concatenate([e2[0:128], e2[128:256] + jnp.where(lom, 0.0, ec)], axis=0)
        l1 = jnp.sum(y1, axis=-1, keepdims=True)
        l2 = jnp.sum(y2, axis=-1, keepdims=True)
        e = jnp.concatenate([e1, e2], axis=1)
        os_ = [lax.dot_general(e[a:b].astype(bf16), bd(sel(vts, Xs[g])), NT, preferred_element_type=f32)
               for g, (a, b) in enumerate(rows)]
        os_[1] = os_[1] + lax.dot_general(ec[0:64].astype(bf16), ev[0], NT, preferred_element_type=f32)
        os_[2] = os_[2] + lax.dot_general(ec[64:128].astype(bf16), ev[1], NT, preferred_element_type=f32)
        o = jnp.concatenate(os_, axis=0)
        l = jnp.where(lo, l1, l2)
        r = pl.reciprocal(l, approx=True)
        r = r * (2.0 - l * r)
        c = (o * r).astype(bf16)
        return jnp.concatenate([c[0:BLK], c[2 * BLK:4 * BLK], c[BLK:2 * BLK]], axis=0)

    def attn_units(units, wq_of, kt_of, vt_of, store):
        s = scores(units[0][-1], wq_of(units[0]), kt_of(units[0]))
        for k, u in enumerate(units):
            if k + 1 < len(units):
                n = units[k + 1]
                s_next = scores(n[-1], wq_of(n), kt_of(n))
            store(u, finish(s, vt_of(u)))
            s = s_next

    def attn(units):
        def store(u, c):
            s, h, b = u
            ctx[b * SQ:(b + 1) * SQ, (2 * s + h) * HALF:(2 * s + h + 1) * HALF] = c
        cache = {}

        def wq_of(u):
            s, h = u[0], u[1]
            if (s, h) not in cache:
                if s == 0:
                    cache[s, h] = wq_o[h]
                else:
                    first = head_q[s - 1] if (s, h) in ((1, A), (2, Bh)) else dec(s, h, U0)
                    cache[s, h] = jnp.concatenate([first, dec(s, h, U1), dec(s, h, U2)], axis=0)
            return cache[s, h]
        attn_units(units, wq_of,
                   lambda u: kt_f[u[0], u[2], u[1] * HALF:(u[1] + 1) * HALF, :],
                   lambda u: vt_f[u[0], u[2], u[1] * HALF:(u[1] + 1) * HALF, :], store)

    def kvwait(P):
        for sh in P:
            for c in c_kv[sh]:
                c.wait()

    def un(P):
        return [(s, h, b) for s, h in P for b in range(B)]

    def swap(v, h, u):
        if h == Bh and u == 1:
            return jnp.concatenate([v[0:128], v[192:256], v[128:192]], axis=0)
        return v

    def own_o(h, u):
        return jnp.concatenate([wo_o[h, 2 * u], wo_o[h, 2 * u + 1]], axis=0)

    def lhs_of(P):
        ks = [2 * s + h for s, h in P]
        return jnp.concatenate([ctx[:, k * HALF:(k + 1) * HALF] for k in ks], axis=1)

    def ocol(lhs, w, c, rsplit=1, first=False):
        for r in range(rsplit):
            rs = slice(r * (ROWS // rsplit), (r + 1) * (ROWS // rsplit))
            o = jnp.dot(lhs[rs], w, preferred_element_type=f32)
            if first:
                out_ref[rs, c * 128:(c + 1) * 128] = o
            else:
                out_ref[rs, c * 128:(c + 1) * 128] += o

    def oproj(P, units=(0, 1), rsplit=1):
        lhs = lhs_of(P)
        for u in units:
            v = [own_o(h, u) if s == 0 else swap(dec(s, h, V0 + u), h, u) for s, h in P]
            for cc in range(2):
                w = jnp.concatenate([t[128 * cc:128 * (cc + 1)] for t in v], axis=0)
                ocol(lhs, w, 2 * u + cc, rsplit, first=P[0][0] == 0)

    P0, P1, P2, P3 = [(0, A), (0, Bh)], [(1, A), (2, Bh)], [(1, Bh), (2, A)], [(3, A), (3, Bh)]
    with scope("own_0"):
        c_x0.wait()
        x_b[0:SQ, :] = x_f[0:SQ, :].astype(bf16)
        for c in c_kv0:
            c.wait()
        attn([(0, A, 0), (0, Bh, 0)])
    with scope("prep_wo"):
        c_wo.wait()
        for h in range(2):
            for c in range(4):
                wo_o[h, c] = wo_f[h * HALF:(h + 1) * HALF, c * 128:(c + 1) * 128].astype(bf16)
        for h in range(2):
            for u in range(2):
                enc(swap(own_o(h, u), h, u), 0, h, V0 + u)
        for d, _, _ in DIRS:
            start(*d["o1"])
    with scope("own_1"):
        c_x1.wait()
        x_b[SQ:2 * SQ, :] = x_f[SQ:2 * SQ, :].astype(bf16)
        for c in c_kv1:
            c.wait()
        attn([(0, A, 1), (0, Bh, 1)])
    with scope("w_q1"):
        for d, slot, h in DIRS:
            d["q0"].wait_recv()
            d["qr"].wait_recv()
            head_q[slot - 1, 0:R0, :] = stage[slot - 1].astype(bf16)
            enc(head_q[slot - 1], slot, h, U0)
            d["u1", h].wait_recv()
            d["u2", h].wait_recv()
            start(*d["fq"], *d["o2"])
    with scope("o_0"):
        oproj(P0)
    with scope("a_1"):
        kvwait(P1)
        attn(un(P1))
    with scope("w_q2"):
        for d, _, h in DIRS:
            for key in (("u1", 1 - h), ("u2", 1 - h), "u0"):
                d[key].wait_recv()
        kvwait(P2)
    with scope("a_2"):
        attn(un(P2))
    with scope("w_o1"):
        for d, _, _ in DIRS:
            for c in d["o1"]:
                c.wait_recv()
            start(*d["fo"])
    with scope("o_1"):
        oproj(P1)
    with scope("w_q3"):
        for d, _, _ in DIRS:
            for c in d["fq"]:
                c.wait_recv()
        kvwait(P3)
    with scope("a_3"):
        attn(un(P3))
    with scope("w_o2"):
        for d, _, _ in DIRS:
            for c in d["o2"]:
                c.wait_recv()
    with scope("o_2"):
        lane = lax.broadcasted_iota(i32, (64, HALF), 1)
        for r in range(4):
            ca = pltpu.bitcast(ctx[r * 128:(r + 1) * 128, 6 * HALF:7 * HALF], i32)
            cb = pltpu.bitcast(ctx[r * 128:(r + 1) * 128, 7 * HALF:8 * HALF], i32)
            t0 = jnp.where(lane < DH, ca, cb)
            t1 = jnp.where(lane < DH, cb, ca)
            if r:
                t0 = pltpu.roll(t0, HALF - 32 * r, 1)
                t1 = pltpu.roll(t1, HALF - 32 * r, 1)
            lhs_t[0, r * 64:(r + 1) * 64, :] = t0
            lhs_t[1, r * 64:(r + 1) * 64, :] = t1
        oproj(P2)
    with scope("w_send0"):
        for d, _, _ in DIRS:
            for key, v in d.items():
                if key != "fo":
                    for c in (v if isinstance(v, list) else [v]):
                        c.wait_send()
    with scope("o_30"):
        R["fo"][0].wait_recv()
        L["fo"][0].wait_recv()
        oproj(P3, units=(0,), rsplit=2)
    with scope("o_32"):
        R["fo"][1].wait_recv()
        L["fo"][1].wait_recv()
        w = jnp.concatenate([dec(3, h, V1, 0, 2) for h in range(2)], axis=0)
        acc = flags[0]
        for f in flags[1:]:
            acc = acc | f
        any_bad = jnp.max(_srl(acc, 31)) > 0
        ocol(lhs_of(P3), w, 2, 4)
    for t in range(2):
        with scope(f"o_4{t}"):
            for d, _, _ in DIRS:
                d["fo"][t].wait_send()
            R["fo"][2 + t].wait_recv()
            L["fo"][2 + t].wait_recv()
            va, vb = dec(3, A, V1, 2 + t, 3 + t), dec(3, Bh, V1, 2 + t, 3 + t)
            w = jnp.concatenate([va, vb] if t == 0 else [vb, va], axis=0)
            for r in range(4):
                wr = w if r == 0 else jnp.concatenate([w[32 * r:128], w[0:32 * r]], axis=0)
                lhs = pltpu.bitcast(lhs_t[t, r * 64:(r + 1) * 64, :], bf16)
                out_ref[r * 128:(r + 1) * 128, 384:512] += jnp.dot(lhs, wr, preferred_element_type=f32)
    for d, _, _ in DIRS:
        d["fo"][2].wait_send()
        d["fo"][3].wait_send()

    @pl.when(any_bad)
    def _():
        cps = []
        for k, (tgt, slot) in enumerate(((right, 1), (left, 2), (diag, 3))):
            for j, (src, dst) in enumerate(((wq_o, raw_q), (wo_o, raw_o))):
                cp = pltpu.make_async_remote_copy(src, dst.at[slot], fsem_s.at[2 * k + j],
                                                  fsem_r.at[2 * k + j],
                                                  device_id=(tgt,), device_id_type=MESH)
                cp.start()
                cps.append(cp)
        raw_q[0] = wq_o[...]
        raw_o[0] = wo_o[...]
        out_ref[...] = jnp.zeros(out_ref.shape, f32)
        for cp in cps:
            cp.wait()

        def piece(t, carry):
            s = t // 2
            h = t % 2
            hs = pl.multiple_of(h * HALF, HALF)

            def store(u, c):
                c_tmp[u[0] * SQ:(u[0] + 1) * SQ, :] = c
            attn_units([(0,), (1,)],
                       lambda u: raw_q[s, h],
                       lambda u: kt_f[s, u[0], pl.ds(hs, HALF), :],
                       lambda u: vt_f[s, u[0], pl.ds(hs, HALF), :], store)
            for c in range(4):
                out_ref[:, c * 128:(c + 1) * 128] += jnp.dot(c_tmp[...], raw_o[s, h, c],
                                                             preferred_element_type=f32)
            return carry
        lax.fori_loop(0, 8, piece, 0)


def pallas_dist_sparse_attn_blocksparse_qseq_b2_sq256_skv256_hq4_dh64_kernel(x, Wq, K_ext, V_ext, Wo):
    x2 = x.reshape(ROWS, DM)
    kt = K_ext.transpose(0, 2, 3, 1).reshape(B, 16 * DH, SKV)
    vt = V_ext.transpose(0, 2, 3, 1).reshape(B, 16 * DH, SKV)
    n_remote = 2 * 18
    out = pl.pallas_call(
        _body,
        out_shape=jax.ShapeDtypeStruct((ROWS, DM), f32),
        in_specs=[pl.BlockSpec(memory_space=pl.ANY)] * 5,
        out_specs=pl.BlockSpec(memory_space=pltpu.VMEM),
        scratch_shapes=[
            pltpu.VMEM((ROWS, DM), f32),
            pltpu.VMEM((ROWS, DM), bf16),
            pltpu.VMEM((DM, 2 * HALF), f32),
            pltpu.VMEM((2 * HALF, DM), f32),
            pltpu.VMEM((2, DM, HALF), bf16),
            pltpu.VMEM((2, 4, HALF, 128), bf16),
            pltpu.VMEM((2, RE, HALF), bf16),
            pltpu.VMEM((4, 2, 5, 104, 128), i32),
            pltpu.VMEM((4, B, 2 * HALF, SKV), f32),
            pltpu.VMEM((4, B, 2 * HALF, SKV), f32),
            pltpu.VMEM((ROWS, 8 * HALF), bf16),
            pltpu.VMEM((2, R0, HALF), f32),
            pltpu.VMEM((ROWS, HALF), bf16),
            pltpu.VMEM((2, ROWS // 2, HALF), i32),
            pltpu.VMEM((4, 2, DM, HALF), bf16),
            pltpu.VMEM((4, 2, 4, HALF, 128), bf16),
            pltpu.SemaphoreType.DMA((4 + 7 + 12,)),
            pltpu.SemaphoreType.DMA((n_remote,)),
            pltpu.SemaphoreType.DMA((n_remote,)),
            pltpu.SemaphoreType.REGULAR((2,)),
            pltpu.SemaphoreType.DMA((6,)),
            pltpu.SemaphoreType.DMA((6,)),
        ],
        compiler_params=pltpu.CompilerParams(collective_id=0,
                                             vmem_limit_bytes=48 * 1024 * 1024,
                                             disable_semaphore_checks=True),
    )(x2, Wq, kt, vt, Wo)
    return out.reshape(B, SQ, DM)
```
